```python
import numpy as np

kernel_name = "dist_mean_ax0_shard0_i_m4096_n1024"

def setup_inputs():
    return {"x": np.random.randn(16384, 1024).astype(np.float32)}

def reference(x: np.ndarray) -> np.ndarray:
    return np.mean(x, axis=0, keepdims=True)
```

```python
import jax
import jax.numpy as jnp
from jax import lax
from jax.experimental import pallas as pl
from jax.experimental.pallas import tpu as pltpu

N_DEV = 4
MESH = pl.DeviceIdType.MESH

CHUNKS = (2528, 768, 128)
TAIL = 256
TAIL_Y = (224, 32)
W = 128
RAW = 208
BLK = 64


def _tree(vals):
    while len(vals) > 1:
        vals = [
            vals[i] + vals[i + 1] if i + 1 < len(vals) else vals[i]
            for i in range(0, len(vals), 2)
        ]
    return vals[0]


def pallas_dist_mean_ax0_shard0_i_m4096_n1024_kernel(x: jax.Array):
    m, n = x.shape
    n_local = m - 2 * RAW
    assert sum(CHUNKS) + TAIL == n_local and sum(TAIL_Y) == TAIL
    inv = 1.0 / (m * N_DEV)
    nch = len(CHUNKS)
    offs = [sum(CHUNKS[:i]) for i in range(nch)]
    toff = sum(CHUNKS)
    yoffs = [toff + sum(TAIL_Y[:i]) for i in range(len(TAIL_Y))]

    def body(x_hbm, o_ref, buf, rbuf, part, recv,
             sems, raw_send, raw_recv, send_sems, recv_sems):
        def local(k, r0, rows, c0, cw):
            cp = pltpu.make_async_copy(
                x_hbm.at[pl.ds(r0, rows), pl.ds(c0, cw)],
                buf.at[pl.ds(r0, rows), pl.ds(c0, cw)],
                sems.at[k])
            cp.start()
            return cp

        copies = [local(c, offs[c], CHUNKS[c], 0, n) for c in range(nch)]
        cx = local(nch, toff, TAIL, W, n - W)
        cys = [local(nch + 1 + y, yoffs[y], TAIL_Y[y], 0, W)
               for y in range(len(TAIL_Y))]

        me = lax.axis_index("i")
        peer = {d: (me + d) & (N_DEV - 1) for d in (1, 2, 3)}
        bar = pltpu.get_barrier_semaphore()
        for d in (2, 1, 3):
            pl.semaphore_signal(bar, inc=1, device_id=(peer[d],),
                                device_id_type=MESH)
        pl.semaphore_wait(bar, N_DEV - 1)

        raws = []
        for l, d in enumerate((1, 3)):
            rd = pltpu.make_async_remote_copy(
                x_hbm.at[pl.ds(n_local + l * RAW, RAW), :], rbuf.at[l],
                raw_send.at[l], raw_recv.at[l],
                device_id=(peer[d],), device_id_type=MESH)
            rd.start()
            raws.append(rd)

        def accum(acc, ref, off, rows, c0=0, cw=n):
            nb, rem = divmod(rows, BLK)
            if nb > 1 and cw == n:
                def step(i, a):
                    r = pl.multiple_of(off + i * BLK, 8)
                    return a + _tree([ref[pl.ds(r + j * 8, 8), :]
                                      for j in range(BLK // 8)])
                acc = lax.fori_loop(0, nb, step, acc)
                off, rows = off + nb * BLK, rem
            if rows:
                acc = acc + _tree([ref[pl.ds(off + j * 8, 8), pl.ds(c0, cw)]
                                   for j in range(rows // 8)])
            return acc

        acc = jnp.zeros((8, n), jnp.float32)
        for c in range(nch):
            copies[c].wait()
            acc = accum(acc, buf, offs[c], CHUNKS[c])
            if c == 1:
                for l in range(2):
                    raws[l].wait_recv()
                    acc = accum(acc, rbuf.at[l], 0, RAW)
                for l in range(2):
                    raws[l].wait_send()

        def send(k, d, c0, cw):
            rd = pltpu.make_async_remote_copy(
                part.at[:, pl.ds(c0, cw)], recv.at[d - 1, :, pl.ds(c0, cw)],
                send_sems.at[k], recv_sems.at[k],
                device_id=(peer[d],), device_id_type=MESH)
            rd.start()
            return rd

        cx.wait()
        a = accum(acc[:, W:], buf, toff, TAIL, W, n - W)
        part[:, pl.ds(W, n - W)] = jnp.sum(a, axis=0, keepdims=True) * inv
        dx = send(0, 2, W, n - W)
        a = acc[:, :W]
        for y in range(len(TAIL_Y)):
            cys[y].wait()
            a = accum(a, buf, yoffs[y], TAIL_Y[y], 0, W)
        part[:, pl.ds(0, W)] = jnp.sum(a, axis=0, keepdims=True) * inv
        dy = send(1, 2, 0, W)
        n1 = send(2, 1, 0, n)
        n3 = send(3, 3, 0, n)
        for rd in (dx, dy, n1, n3):
            rd.wait_send()

        n1.wait_recv()
        n3.wait_recv()
        sx, sy = pl.ds(W, n - W), pl.ds(0, W)
        tx = part[:, sx] + recv[0, :, sx] + recv[2, :, sx]
        ty = part[:, sy] + recv[0, :, sy] + recv[2, :, sy]
        dx.wait_recv()
        o_ref[:, sx] = tx + recv[1, :, sx]
        dy.wait_recv()
        o_ref[:, sy] = ty + recv[1, :, sy]

    return pl.pallas_call(
        body,
        out_shape=jax.ShapeDtypeStruct((1, n), jnp.float32),
        in_specs=[pl.BlockSpec(memory_space=pl.ANY)],
        out_specs=pl.BlockSpec(memory_space=pltpu.VMEM),
        scratch_shapes=[
            pltpu.VMEM((n_local, n), jnp.float32),
            pltpu.VMEM((2, RAW, n), jnp.float32),
            pltpu.VMEM((1, n), jnp.float32),
            pltpu.VMEM((N_DEV - 1, 1, n), jnp.float32),
            pltpu.SemaphoreType.DMA((nch + 1 + len(TAIL_Y),)),
            pltpu.SemaphoreType.DMA((2,)),
            pltpu.SemaphoreType.DMA((2,)),
            pltpu.SemaphoreType.DMA((4,)),
            pltpu.SemaphoreType.DMA((4,)),
        ],
        compiler_params=pltpu.CompilerParams(
            collective_id=0,
            vmem_limit_bytes=40 * 1024 * 1024,
            disable_semaphore_checks=True,
        ),
    )(x)
```

```python
import jax
import jax.numpy as jnp
from jax import lax
from jax.experimental import pallas as pl
from jax.experimental.pallas import tpu as pltpu

N_DEV = 4
MESH = pl.DeviceIdType.MESH

CHUNKS = (2512, 768, 128)
TAIL_X = (224, 32)
TAIL_Y = (224, 32)
W = 128
RAWS = (200, 16)
BLK = 64


def _offsets(sizes, base=0):
    return [base + sum(sizes[:i]) for i in range(len(sizes))]


def _tree(vals):
    while len(vals) > 1:
        vals = [
            vals[i] + vals[i + 1] if i + 1 < len(vals) else vals[i]
            for i in range(0, len(vals), 2)
        ]
    return vals[0]


def _accum(acc, ref, off, rows, c0, cw):
    cols = pl.ds(c0, cw)
    nb, rem = divmod(rows, BLK)
    if nb > 1 and cw > W:
        def step(i, a):
            blk = ref[pl.ds(pl.multiple_of(off + i * BLK, 8), BLK), cols]
            return a + _tree([blk[j * 8:(j + 1) * 8] for j in range(BLK // 8)])

        acc = lax.fori_loop(0, nb, step, acc)
        off, rows = off + nb * BLK, rem
    if rows:
        acc = acc + _tree(
            [ref[pl.ds(off + j * 8, 8), cols] for j in range(rows // 8)])
    return acc


def pallas_dist_mean_ax0_shard0_i_m4096_n1024_kernel(x: jax.Array):
    m, n = x.shape
    raw, tail = sum(RAWS), sum(TAIL_X)
    n_local = m - 2 * raw
    toff = sum(CHUNKS)
    assert toff + tail == n_local and sum(TAIL_Y) == tail
    inv = 1.0 / (m * N_DEV)
    coffs = _offsets(CHUNKS)
    xoffs = _offsets(TAIL_X, toff)
    yoffs = _offsets(TAIL_Y)
    roffs = _offsets(RAWS)
    n_loc_dma = len(CHUNKS) + len(TAIL_X) + len(TAIL_Y)
    sx, sy = pl.ds(W, n - W), pl.ds(0, W)

    def body(x_hbm, o_ref, buf, ybuf, rbuf, part, recv,
             sems, raw_send, raw_recv, send_sems, recv_sems):
        n_started = [0]

        def fetch(src, dst):
            cp = pltpu.make_async_copy(src, dst, sems.at[n_started[0]])
            cp.start()
            n_started[0] += 1
            return cp

        chunks = [
            fetch(x_hbm.at[pl.ds(o, r), :], buf.at[pl.ds(o, r), :])
            for o, r in zip(coffs, CHUNKS)]
        cxs = [
            fetch(x_hbm.at[pl.ds(o, r), sx], buf.at[pl.ds(o, r), sx])
            for o, r in zip(xoffs, TAIL_X)]
        cys = [
            fetch(x_hbm.at[pl.ds(toff + o, r), sy], ybuf.at[pl.ds(o, r), :])
            for o, r in zip(yoffs, TAIL_Y)]

        me = lax.axis_index("i")
        peer = {d: (me + d) & (N_DEV - 1) for d in (1, 2, 3)}
        bar = pltpu.get_barrier_semaphore()
        for d in (2, 1, 3):
            pl.semaphore_signal(
                bar, inc=1, device_id=(peer[d],), device_id_type=MESH)
        pl.semaphore_wait(bar, N_DEV - 1)

        raws = {}
        for s, (o, r) in enumerate(zip(roffs, RAWS)):
            for l, d in enumerate((1, 3)):
                rd = pltpu.make_async_remote_copy(
                    x_hbm.at[pl.ds(n_local + l * raw + o, r), :],
                    rbuf.at[l, pl.ds(o, r), :],
                    raw_send.at[2 * s + l], raw_recv.at[2 * s + l],
                    device_id=(peer[d],), device_id_type=MESH)
                rd.start()
                raws[s, l] = rd

        acc = jnp.zeros((8, n), jnp.float32)
        for cp, o, r in zip(chunks, coffs, CHUNKS):
            cp.wait()
            acc = _accum(acc, buf, o, r, 0, n)
        for l in range(2):
            raws[0, l].wait_recv()
            acc = _accum(acc, rbuf.at[l], roffs[0], RAWS[0], 0, n)

        def send(k, d, cols):
            rd = pltpu.make_async_remote_copy(
                part.at[:, cols], recv.at[d - 1, :, cols],
                send_sems.at[k], recv_sems.at[k],
                device_id=(peer[d],), device_id_type=MESH)
            rd.start()
            return rd

        ax, ay = acc[:, W:], acc[:, :W]
        cxs[0].wait()
        ax = _accum(ax, buf, xoffs[0], TAIL_X[0], W, n - W)
        for l in range(2):
            raws[1, l].wait_recv()
            ax = _accum(ax, rbuf.at[l], roffs[1], RAWS[1], W, n - W)
            ay = _accum(ay, rbuf.at[l], roffs[1], RAWS[1], 0, W)
        cxs[1].wait()
        ax = _accum(ax, buf, xoffs[1], TAIL_X[1], W, n - W)
        part[:, sx] = jnp.sum(ax, axis=0, keepdims=True) * inv
        far_x = send(0, 2, sx)
        for cp, o, r in zip(cys, yoffs, TAIL_Y):
            cp.wait()
            ay = _accum(ay, ybuf, o, r, 0, W)
        part[:, sy] = jnp.sum(ay, axis=0, keepdims=True) * inv
        far_y = send(1, 2, sy)
        near_r = send(2, 1, pl.ds(0, n))
        near_l = send(3, 3, pl.ds(0, n))
        for rd in list(raws.values()) + [far_x, far_y, near_r, near_l]:
            rd.wait_send()

        near_r.wait_recv()
        near_l.wait_recv()
        tx = part[:, sx] + recv[0, :, sx] + recv[2, :, sx]
        ty = part[:, sy] + recv[0, :, sy] + recv[2, :, sy]
        far_x.wait_recv()
        o_ref[:, sx] = tx + recv[1, :, sx]
        far_y.wait_recv()
        o_ref[:, sy] = ty + recv[1, :, sy]

    params = dict(collective_id=0, vmem_limit_bytes=32 * 1024 * 1024)
    if hasattr(pltpu.CompilerParams, "disable_semaphore_checks"):
        params["disable_semaphore_checks"] = True

    return pl.pallas_call(
        body,
        out_shape=jax.ShapeDtypeStruct((1, n), jnp.float32),
        in_specs=[pl.BlockSpec(memory_space=pl.ANY)],
        out_specs=pl.BlockSpec(memory_space=pltpu.VMEM),
        scratch_shapes=[
            pltpu.VMEM((n_local, n), jnp.float32),
            pltpu.VMEM((tail, W), jnp.float32),
            pltpu.VMEM((2, raw, n), jnp.float32),
            pltpu.VMEM((1, n), jnp.float32),
            pltpu.VMEM((N_DEV - 1, 1, n), jnp.float32),
            pltpu.SemaphoreType.DMA((n_loc_dma,)),
            pltpu.SemaphoreType.DMA((2 * len(RAWS),)),
            pltpu.SemaphoreType.DMA((2 * len(RAWS),)),
            pltpu.SemaphoreType.DMA((4,)),
            pltpu.SemaphoreType.DMA((4,)),
        ],
        compiler_params=pltpu.CompilerParams(**params),
    )(x)
```

```python
import jax
import jax.numpy as jnp
from jax import lax
from jax.experimental import pallas as pl
from jax.experimental.pallas import tpu as pltpu

N_DEV = 4
MESH = pl.DeviceIdType.MESH

CHUNKS = (2416, 768, 128)
TAIL_X = (224, 32)
TAIL_Y = (224, 32)
W = 128
RAWS = (200, 16)
VIA_SMEM = 96
BLK = 64


def _offsets(sizes, base=0):
    return [base + sum(sizes[:i]) for i in range(len(sizes))]


def _tree(vals):
    while len(vals) > 1:
        vals = [
            vals[i] + vals[i + 1] if i + 1 < len(vals) else vals[i]
            for i in range(0, len(vals), 2)
        ]
    return vals[0]


def _accum(acc, ref, off, rows, c0, cw):
    cols = pl.ds(c0, cw)
    nb, rem = divmod(rows, BLK)
    if nb > 1 and cw > W:
        def step(i, a):
            blk = ref[pl.ds(pl.multiple_of(off + i * BLK, 8), BLK), cols]
            return a + _tree([blk[j * 8:(j + 1) * 8] for j in range(BLK // 8)])

        acc = lax.fori_loop(0, nb, step, acc)
        off, rows = off + nb * BLK, rem
    if rows:
        acc = acc + _tree(
            [ref[pl.ds(off + j * 8, 8), cols] for j in range(rows // 8)])
    return acc


def pallas_dist_mean_ax0_shard0_i_m4096_n1024_kernel(x: jax.Array):
    m, n = x.shape
    raw, tail = sum(RAWS), sum(TAIL_X)
    n_local = m - 2 * raw - VIA_SMEM
    toff = sum(CHUNKS)
    assert toff + tail == n_local and sum(TAIL_Y) == tail
    inv = 1.0 / (m * N_DEV)
    coffs = _offsets(CHUNKS)
    xoffs = _offsets(TAIL_X, toff)
    yoffs = _offsets(TAIL_Y)
    roffs = _offsets(RAWS)
    n_loc_dma = len(CHUNKS) + len(TAIL_X) + len(TAIL_Y) + 2
    sx, sy = pl.ds(W, n - W), pl.ds(0, W)

    def body(x_hbm, o_ref, buf, ybuf, rbuf, sbuf, vbuf, part, recv,
             sems, raw_send, raw_recv, send_sems, recv_sems):
        n_started = [0]

        def fetch(src, dst):
            cp = pltpu.make_async_copy(src, dst, sems.at[n_started[0]])
            cp.start()
            n_started[0] += 1
            return cp

        chunks = [
            fetch(x_hbm.at[pl.ds(o, r), :], buf.at[pl.ds(o, r), :])
            for o, r in zip(coffs, CHUNKS)]
        to_smem = fetch(x_hbm.at[pl.ds(m - VIA_SMEM, VIA_SMEM), :], sbuf)
        cxs = [
            fetch(x_hbm.at[pl.ds(o, r), sx], buf.at[pl.ds(o, r), sx])
            for o, r in zip(xoffs, TAIL_X)]
        cys = [
            fetch(x_hbm.at[pl.ds(toff + o, r), sy], ybuf.at[pl.ds(o, r), :])
            for o, r in zip(yoffs, TAIL_Y)]

        me = lax.axis_index("i")
        peer = {d: (me + d) & (N_DEV - 1) for d in (1, 2, 3)}
        bar = pltpu.get_barrier_semaphore()
        for d in (2, 1, 3):
            pl.semaphore_signal(
                bar, inc=1, device_id=(peer[d],), device_id_type=MESH)
        pl.semaphore_wait(bar, N_DEV - 1)

        raws = {}
        for s, (o, r) in enumerate(zip(roffs, RAWS)):
            for l, d in enumerate((1, 3)):
                rd = pltpu.make_async_remote_copy(
                    x_hbm.at[pl.ds(n_local + l * raw + o, r), :],
                    rbuf.at[l, pl.ds(o, r), :],
                    raw_send.at[2 * s + l], raw_recv.at[2 * s + l],
                    device_id=(peer[d],), device_id_type=MESH)
                rd.start()
                raws[s, l] = rd

        to_smem.wait()
        from_smem = fetch(sbuf, vbuf)

        acc = jnp.zeros((8, n), jnp.float32)
        for cp, o, r in zip(chunks, coffs, CHUNKS):
            cp.wait()
            acc = _accum(acc, buf, o, r, 0, n)
        for l in range(2):
            raws[0, l].wait_recv()
            acc = _accum(acc, rbuf.at[l], roffs[0], RAWS[0], 0, n)
        from_smem.wait()
        acc = _accum(acc, vbuf, 0, VIA_SMEM, 0, n)

        def send(k, d, cols):
            rd = pltpu.make_async_remote_copy(
                part.at[:, cols], recv.at[d - 1, :, cols],
                send_sems.at[k], recv_sems.at[k],
                device_id=(peer[d],), device_id_type=MESH)
            rd.start()
            return rd

        ax, ay = acc[:, W:], acc[:, :W]
        cxs[0].wait()
        ax = _accum(ax, buf, xoffs[0], TAIL_X[0], W, n - W)
        for l in range(2):
            raws[1, l].wait_recv()
            ax = _accum(ax, rbuf.at[l], roffs[1], RAWS[1], W, n - W)
            ay = _accum(ay, rbuf.at[l], roffs[1], RAWS[1], 0, W)
        cxs[1].wait()
        ax = _accum(ax, buf, xoffs[1], TAIL_X[1], W, n - W)
        part[:, sx] = jnp.sum(ax, axis=0, keepdims=True) * inv
        far_x = send(0, 2, sx)
        for cp, o, r in zip(cys, yoffs, TAIL_Y):
            cp.wait()
            ay = _accum(ay, ybuf, o, r, 0, W)
        part[:, sy] = jnp.sum(ay, axis=0, keepdims=True) * inv
        far_y = send(1, 2, sy)
        near_r = send(2, 1, pl.ds(0, n))
        near_l = send(3, 3, pl.ds(0, n))
        for rd in list(raws.values()) + [far_x, far_y, near_r, near_l]:
            rd.wait_send()

        near_r.wait_recv()
        near_l.wait_recv()
        tx = part[:, sx] + recv[0, :, sx] + recv[2, :, sx]
        ty = part[:, sy] + recv[0, :, sy] + recv[2, :, sy]
        far_x.wait_recv()
        o_ref[:, sx] = tx + recv[1, :, sx]
        far_y.wait_recv()
        o_ref[:, sy] = ty + recv[1, :, sy]

    params = dict(collective_id=0, vmem_limit_bytes=32 * 1024 * 1024)
    if hasattr(pltpu.CompilerParams, "disable_semaphore_checks"):
        params["disable_semaphore_checks"] = True

    return pl.pallas_call(
        body,
        out_shape=jax.ShapeDtypeStruct((1, n), jnp.float32),
        in_specs=[pl.BlockSpec(memory_space=pl.ANY)],
        out_specs=pl.BlockSpec(memory_space=pltpu.VMEM),
        scratch_shapes=[
            pltpu.VMEM((n_local, n), jnp.float32),
            pltpu.VMEM((tail, W), jnp.float32),
            pltpu.VMEM((2, raw, n), jnp.float32),
            pltpu.SMEM((VIA_SMEM, n), jnp.float32),
            pltpu.VMEM((VIA_SMEM, n), jnp.float32),
            pltpu.VMEM((1, n), jnp.float32),
            pltpu.VMEM((N_DEV - 1, 1, n), jnp.float32),
            pltpu.SemaphoreType.DMA((n_loc_dma,)),
            pltpu.SemaphoreType.DMA((2 * len(RAWS),)),
            pltpu.SemaphoreType.DMA((2 * len(RAWS),)),
            pltpu.SemaphoreType.DMA((4,)),
            pltpu.SemaphoreType.DMA((4,)),
        ],
        compiler_params=pltpu.CompilerParams(**params),
    )(x)
```

```python
import jax
import jax.numpy as jnp
from jax import lax
from jax.experimental import pallas as pl
from jax.experimental.pallas import tpu as pltpu

N_DEV = 4
MESH = pl.DeviceIdType.MESH

CHUNKS = (2512, 768, 128)
TAIL_X = (224, 32)
TAIL_Y = (224, 32)
W = 128
RAWS = (200, 16)
BLK = 64


def _offsets(sizes, base=0):
    return [base + sum(sizes[:i]) for i in range(len(sizes))]


def _tree(vals):
    while len(vals) > 1:
        vals = [
            vals[i] + vals[i + 1] if i + 1 < len(vals) else vals[i]
            for i in range(0, len(vals), 2)
        ]
    return vals[0]


def _accum(acc, ref, off, rows, c0, cw):
    cols = pl.ds(c0, cw)
    nb, rem = divmod(rows, BLK)
    if nb > 1 and cw > W:
        def step(i, a):
            blk = ref[pl.ds(pl.multiple_of(off + i * BLK, 8), BLK), cols]
            return a + _tree([blk[j * 8:(j + 1) * 8] for j in range(BLK // 8)])

        acc = lax.fori_loop(0, nb, step, acc)
        off, rows = off + nb * BLK, rem
    if rows:
        acc = acc + _tree(
            [ref[pl.ds(off + j * 8, 8), cols] for j in range(rows // 8)])
    return acc


def pallas_dist_mean_ax0_shard0_i_m4096_n1024_kernel(x: jax.Array):
    m, n = x.shape
    raw, tail = sum(RAWS), sum(TAIL_X)
    n_local = m - 2 * raw
    toff = sum(CHUNKS)
    assert toff + tail == n_local and sum(TAIL_Y) == tail
    inv = 1.0 / (m * N_DEV)
    coffs = _offsets(CHUNKS)
    xoffs = _offsets(TAIL_X, toff)
    yoffs = _offsets(TAIL_Y)
    roffs = _offsets(RAWS)
    n_fetch = len(CHUNKS) + len(TAIL_X) + len(TAIL_Y)
    n_push = 2 * len(RAWS) + 4
    sx, sy = pl.ds(W, n - W), pl.ds(0, W)

    def body(x_hbm, o_ref, buf, ybuf, rbuf, px, py, part, near, farx, fary):

        def scoped(fetch_sems, send_sems, recv_sems):
            fetches = []

            def fetch(src, dst):
                cp = pltpu.make_async_copy(
                    src, dst, fetch_sems.at[len(fetches)])
                cp.start()
                fetches.append(cp)
                return cp

            chunks = [
                fetch(x_hbm.at[pl.ds(o, r), :], buf.at[pl.ds(o, r), :])
                for o, r in zip(coffs, CHUNKS)]
            cxs = [
                fetch(x_hbm.at[pl.ds(o, r), sx], buf.at[pl.ds(o, r), sx])
                for o, r in zip(xoffs, TAIL_X)]
            cys = [
                fetch(x_hbm.at[pl.ds(toff + o, r), sy],
                      ybuf.at[pl.ds(o, r), :])
                for o, r in zip(yoffs, TAIL_Y)]

            me = lax.axis_index("i")
            peer = {d: (me + d) & (N_DEV - 1) for d in (1, 2, 3)}
            bar = pltpu.get_barrier_semaphore()
            for d in (2, 1, 3):
                pl.semaphore_signal(
                    bar, inc=1, device_id=(peer[d],), device_id_type=MESH)
            pl.semaphore_wait(bar, N_DEV - 1)

            pushes = []

            def push(src, dst, d):
                k = len(pushes)
                rd = pltpu.make_async_remote_copy(
                    src, dst, send_sems.at[k], recv_sems.at[k],
                    device_id=(peer[d],), device_id_type=MESH)
                rd.start()
                pushes.append(rd)
                return rd

            raws = [
                [push(x_hbm.at[pl.ds(n_local + l * raw + o, r), :],
                      rbuf.at[l, pl.ds(o, r), :], d)
                 for l, d in enumerate((1, 3))]
                for o, r in zip(roffs, RAWS)]

            acc = jnp.zeros((8, n), jnp.float32)
            for cp, o, r in zip(chunks, coffs, CHUNKS):
                cp.wait()
                acc = _accum(acc, buf, o, r, 0, n)
            for l in range(2):
                raws[0][l].wait_recv()
                acc = _accum(acc, rbuf.at[l], roffs[0], RAWS[0], 0, n)

            ax, ay = acc[:, W:], acc[:, :W]
            cxs[0].wait()
            ax = _accum(ax, buf, xoffs[0], TAIL_X[0], W, n - W)
            for l in range(2):
                raws[1][l].wait_recv()
                ax = _accum(ax, rbuf.at[l], roffs[1], RAWS[1], W, n - W)
                ay = _accum(ay, rbuf.at[l], roffs[1], RAWS[1], 0, W)
            cxs[1].wait()
            ax = _accum(ax, buf, xoffs[1], TAIL_X[1], W, n - W)
            mx = jnp.sum(ax, axis=0, keepdims=True) * inv
            px[...] = mx
            far_x = push(px, farx, 2)
            part[:, sx] = mx
            for cp, o, r in zip(cys, yoffs, TAIL_Y):
                cp.wait()
                ay = _accum(ay, ybuf, o, r, 0, W)
            my = jnp.sum(ay, axis=0, keepdims=True) * inv
            py[...] = my
            far_y = push(py, fary, 2)
            part[:, sy] = my
            near_r = push(part, near.at[0], 1)
            near_l = push(part, near.at[1], 3)
            for rd in pushes:
                rd.wait_send()

            near_r.wait_recv()
            near_l.wait_recv()
            tx = part[:, sx] + near[0, :, sx] + near[1, :, sx]
            ty = part[:, sy] + near[0, :, sy] + near[1, :, sy]
            far_x.wait_recv()
            o_ref[:, sx] = tx + farx[...]
            far_y.wait_recv()
            o_ref[:, sy] = ty + fary[...]

        pl.run_scoped(
            scoped,
            pltpu.SemaphoreType.DMA((n_fetch,)),
            pltpu.SemaphoreType.DMA((n_push,)),
            pltpu.SemaphoreType.DMA((n_push,)),
        )

    return pl.pallas_call(
        body,
        out_shape=jax.ShapeDtypeStruct((1, n), jnp.float32),
        in_specs=[pl.BlockSpec(memory_space=pl.ANY)],
        out_specs=pl.BlockSpec(memory_space=pltpu.VMEM),
        scratch_shapes=[
            pltpu.VMEM((n_local, n), jnp.float32),
            pltpu.VMEM((tail, W), jnp.float32),
            pltpu.VMEM((2, raw, n), jnp.float32),
            pltpu.VMEM((1, n - W), jnp.float32),
            pltpu.VMEM((1, W), jnp.float32),
            pltpu.VMEM((1, n), jnp.float32),
            pltpu.VMEM((2, 1, n), jnp.float32),
            pltpu.VMEM((1, n - W), jnp.float32),
            pltpu.VMEM((1, W), jnp.float32),
        ],
        compiler_params=pltpu.CompilerParams(
            collective_id=0, vmem_limit_bytes=32 * 1024 * 1024),
    )(x)
```
